```python
import numpy as np

kernel_name = "dist_moe_shared_ep_outshard_n256_d128_e2_h256"

def setup_inputs():
    x = np.random.randn(256, 128).astype(np.float32)
    router_W = np.random.randn(128, 8).astype(np.float32) * 0.1
    scores64 = x.astype(np.float64) @ router_W.astype(np.float64)
    route_idx = np.argsort(-scores64, axis=-1)[:, :1].astype(np.int32)
    expert_W = np.random.randn(8, 128, 256).astype(np.float32) * 0.02
    shared_W = np.random.randn(128, 256).astype(np.float32) * 0.02
    return {"x": x, "router_W": router_W, "route_idx": route_idx, "expert_W": expert_W, "shared_W": shared_W}

def reference(x, router_W, route_idx, expert_W, shared_W):
    scores = x @ router_W
    s_max = scores.max(axis=-1, keepdims=True)
    probs = np.exp(scores - s_max)
    probs = probs / probs.sum(axis=-1, keepdims=True)
    shared = x @ shared_W
    out = np.zeros((256, 256), dtype=np.float32)
    for i in range(256):
        e = int(route_idx[i, 0])
        out[i] = shared[i] + probs[i, e] * (x[i] @ expert_W[e])
    return out
```

```python
import contextlib
import jax
import jax.numpy as jnp
from jax import lax
from jax.experimental import pallas as pl
from jax.experimental.pallas import tpu as pltpu

N_DEV = 4
MESH = pl.DeviceIdType.MESH


def make(checks=False, split=2, order="rwx", wmode="pow2", scopes=False, pk="bits", ksplit=1):
    sc = (lambda n: jax.named_scope(n)) if scopes else (lambda n: contextlib.nullcontext())

    def fn(x, router_W, route_idx, expert_W, shared_W):
        T, D = x.shape
        E_loc, _, H = expert_W.shape
        E = router_W.shape[1]
        R = T // N_DEV
        HH = H // 2

        def pack(lo, hi):
            if pk == "elem":
                return pltpu.pack_elementwise([lo, hi], packed_dtype=jnp.bfloat16)
            lo = lo.astype(jnp.bfloat16).astype(jnp.float32)
            hi = hi.astype(jnp.bfloat16).astype(jnp.float32)
            lo = lax.bitcast_convert_type(lo, jnp.uint32)
            hi = lax.bitcast_convert_type(hi, jnp.uint32)
            return hi | (lo >> 16)

        def unpack(w):
            lo = lax.bitcast_convert_type(w << 16, jnp.float32)
            hi = lax.bitcast_convert_type(w & jnp.uint32(0xFFFF0000), jnp.float32)
            return lo, hi

        def body(x_hbm, rw_hbm, ri_hbm, ew_hbm, sw_hbm, o_ref,
                 xv, ewv, swv, rwv, riv, send_buf, recv_buf, ld_sems, send_sem, recv_sem):
            sem_ids = iter(range(16))

            def ld(src, dst):
                c = pltpu.make_async_copy(src, dst, ld_sems.at[next(sem_ids)])
                c.start()
                return c

            def ld_w(e):
                c = D // ksplit
                return [ld(ew_hbm.at[e, pl.ds(j * c, c)], ewv.at[e, pl.ds(j * c, c)]) for j in reversed(range(ksplit))]

            for ch in order:
                if ch == "r": c_ri = ld(ri_hbm, riv)
                if ch == "w": c_w = [ld_w(0)]
                if ch == "x": c_x0 = ld(x_hbm.at[pl.ds(0, R)], xv.at[pl.ds(0, R)])
            c_w.append(ld_w(1))
            c_xr = ld(x_hbm.at[pl.ds(R, T - R)], xv.at[pl.ds(R, T - R)])
            c_rest = [ld(sw_hbm, swv), ld(rw_hbm, rwv)]

            me = lax.axis_index("i")
            bar = pltpu.get_barrier_semaphore()
            for k in range(1, N_DEV):
                pl.semaphore_signal(bar, inc=1, device_id=((me + k) & (N_DEV - 1),), device_id_type=MESH)

            sub = lax.broadcasted_iota(jnp.int32, (8, 128), 0)
            lane = lax.broadcasted_iota(jnp.int32, (8, 128), 1)
            bit = (jnp.int32(1) << (15 - (lane & 15))).astype(jnp.float32)
            in_word = (lane >> 5) == (sub >> 1)
            bit_a = jnp.where(in_word & ((lane & 16) == 0), bit, 0.0)
            bit_b = jnp.where(in_word & ((lane & 16) != 0), bit, 0.0)
            want = me * E_loc + (sub & 1)
            with sc("w_ri"):
                c_ri.wait()
            words = [[] for _ in range(E_loc)]
            for h in range(T // 128):
                hit = (jnp.broadcast_to(riv[:, pl.ds(128 * h, 128)], (8, 128)) & (E - 1)) == want
                a = jnp.sum(jnp.where(hit, bit_a, 0.0), axis=1, keepdims=True).astype(jnp.int32)
                b = jnp.sum(jnp.where(hit, bit_b, 0.0), axis=1, keepdims=True).astype(jnp.int32)
                wv = (a << 16) | b
                for s in range(8):
                    words[s & 1].append(wv[s, 0])

            def for_bits(m0, f):
                def step(m):
                    j = lax.clz(m)
                    f(j)
                    return m ^ lax.shift_right_logical(jnp.int32(-2**31), j)
                lax.while_loop(lambda m: m != 0, step, m0)

            def send(k, e):
                for w in range(2):
                    def f(j):
                        pltpu.make_async_remote_copy(
                            src_ref=send_buf.at[pl.ds(e * T + k * R + 32 * w + j, 1)],
                            dst_ref=recv_buf.at[pl.ds(32 * w + j, 1)],
                            send_sem=send_sem, recv_sem=recv_sem,
                            device_id=(k,), device_id_type=MESH).start()
                    for_bits(jnp.where(me == k, 0, words[e][2 * k + w]), f)

            def keep(e):
                for w in range(2):
                    m0 = words[e][w]
                    for k in range(1, N_DEV):
                        m0 = jnp.where(me == k, words[e][2 * k + w], m0)
                    def f(j):
                        pltpu.make_async_copy(
                            send_buf.at[pl.ds(e * T + me * R + 32 * w + j, 1)],
                            recv_buf.at[pl.ds(32 * w + j, 1)], recv_sem).start()
                    for_bits(m0, f)

            @pl.when(me != 0)
            def _():
                pl.semaphore_wait(bar, N_DEV - 1)
            with sc("w_x0"):
                c_x0.wait()
            c = R // split
            xs = [xv[pl.ds(j * c, c), :].astype(jnp.bfloat16) for j in range(split)]
            for e in range(E_loc):
                wl, wh = [], []
                kc = D // ksplit
                for i, j in enumerate(reversed(range(ksplit))):
                    if i == ksplit - 1:
                        with sc(f"w_w{e}"):
                            c_w[e][i].wait()
                    else:
                        c_w[e][i].wait()
                    wl.insert(0, ewv[e, pl.ds(j * kc, kc), pl.ds(0, HH)].astype(jnp.bfloat16))
                    wh.insert(0, ewv[e, pl.ds(j * kc, kc), pl.ds(HH, HH)].astype(jnp.bfloat16))
                wl = jnp.concatenate(wl, axis=0)
                wh = jnp.concatenate(wh, axis=0)
                for j in range(split):
                    lo = jnp.dot(xs[j], wl, preferred_element_type=jnp.float32)
                    hi = jnp.dot(xs[j], wh, preferred_element_type=jnp.float32)
                    send_buf[pl.ds(e * T + j * c, c), :] = pack(lo, hi)
                with sc(f"send{e}"):
                    send(0, e)

            c_xr.wait()
            xr = xv[pl.ds(R, T - R), :].astype(jnp.bfloat16)
            for e in range(E_loc):
                y = jnp.dot(xr, ewv[e].astype(jnp.bfloat16), preferred_element_type=jnp.float32)
                send_buf[pl.ds(e * T + R, T - R), :] = pack(y[:, :HH], y[:, HH:])

            for c_ in c_rest:
                c_.wait()
            xo = xv[pl.ds(pl.multiple_of(me * R, R), R), :].astype(jnp.bfloat16)
            sh = jnp.dot(xo, swv[...].astype(jnp.bfloat16), preferred_element_type=jnp.float32)
            s = lax.dot_general(xo, rwv[...].astype(jnp.bfloat16), (((1,), (1,)), ((), ())), preferred_element_type=jnp.float32)
            p = jnp.exp(s - jnp.max(s, axis=-1, keepdims=True))
            rv = jnp.broadcast_to(riv[...] & (E - 1), (R, T)).astype(jnp.float32)
            mine = lax.broadcasted_iota(jnp.int32, (R, T), 1) == lax.broadcasted_iota(jnp.int32, (R, T), 0) + me * R
            rcol = jnp.sum(jnp.where(mine, rv, 0.0), axis=-1, keepdims=True)
            oh = lax.broadcasted_iota(jnp.int32, s.shape, 1).astype(jnp.float32) == rcol
            psel = jnp.sum(jnp.where(oh, p, 0.0), axis=-1, keepdims=True) / jnp.sum(p, axis=-1, keepdims=True)
            psel = jnp.broadcast_to(psel, (R, HH))

            rr = riv[...] & (E - 1)
            tok = lax.broadcasted_iota(jnp.int32, (1, T), 1)
            n = jnp.sum(jnp.where(((rr >> 1) == me) & ((tok >> 6) != me), 1.0, 0.0)).astype(jnp.int32)

            @pl.when(me == 0)
            def _():
                pl.semaphore_wait(bar, N_DEV - 1)
            with sc("send_nb"):
                for k in (1, 3, 2):
                    for e in range(E_loc):
                        send(k, e)
            for e in range(E_loc):
                keep(e)

            def wait_rows(c):
                v = send_buf.at[pl.ds(0, c)]
                pltpu.make_async_copy(v, v, send_sem).wait()
            if wmode == "fori":
                lax.fori_loop(0, n, lambda j, _: wait_rows(1), None)
            elif wmode == "pow2":
                for b in reversed(range(8)):
                    pl.when((n & (1 << b)) != 0)(lambda b=b: wait_rows(1 << b))

            with sc("w_recv"):
                pltpu.make_async_copy(recv_buf, recv_buf, recv_sem).wait()
            lo, hi = unpack(recv_buf[...])
            o_ref[:, :HH] = sh[:, :HH] + psel * lo
            o_ref[:, HH:] = sh[:, HH:] + psel * hi

        hb = pl.BlockSpec(memory_space=pltpu.HBM)
        ins = (x, router_W.T, route_idx.reshape(1, T), expert_W, shared_W)
        ins = tuple(pltpu.with_memory_space_constraint(a, pltpu.HBM) for a in ins)
        return pl.pallas_call(
            body,
            out_shape=jax.ShapeDtypeStruct((R, H), jnp.float32),
            in_specs=[hb] * 5,
            out_specs=pl.BlockSpec(memory_space=pltpu.VMEM),
            scratch_shapes=[
                pltpu.VMEM((T, D), jnp.float32),
                pltpu.VMEM((E_loc, D, H), jnp.float32),
                pltpu.VMEM((D, H), jnp.float32),
                pltpu.VMEM((E, D), jnp.float32),
                pltpu.VMEM((1, T), jnp.int32),
                pltpu.VMEM((E_loc * T, HH), jnp.uint32),
                pltpu.VMEM((R, HH), jnp.uint32),
                pltpu.SemaphoreType.DMA((5 + 2 * ksplit,)),
                pltpu.SemaphoreType.DMA,
                pltpu.SemaphoreType.DMA,
            ],
            compiler_params=pltpu.CompilerParams(collective_id=0, disable_bounds_checks=not checks, disable_semaphore_checks=not checks),
        )(*ins)
    return fn


pallas_dist_moe_shared_ep_outshard_n256_d128_e2_h256_kernel = make()
```

```python
import functools

import jax
import jax.numpy as jnp
from jax import lax
from jax.experimental import pallas as pl
from jax.experimental.pallas import tpu as pltpu

N_DEV = 4
N_LOCAL = 2
WORD = 32
MESH = pl.DeviceIdType.MESH


def _mm(a, b):
    return jnp.dot(
        a.astype(jnp.bfloat16),
        b.astype(jnp.bfloat16),
        preferred_element_type=jnp.float32,
    )


def _pack(y):
    half = y.shape[1] // 2
    lo, hi = (
        lax.bitcast_convert_type(
            v.astype(jnp.bfloat16).astype(jnp.float32), jnp.uint32
        )
        for v in (y[:, :half], y[:, half:])
    )
    return hi | (lo >> 16)


def _unpack(w):
    lo = lax.bitcast_convert_type(w << 16, jnp.float32)
    hi = lax.bitcast_convert_type(w & jnp.uint32(0xFFFF0000), jnp.float32)
    return lo, hi


def _pop_rows(masks):
    tops = [lax.clz(m) & (WORD - 1) for m in masks]
    found = [(m != 0, WORD * w + j) for w, (m, j) in enumerate(zip(masks, tops))]
    rest = tuple(
        m & lax.shift_right_logical(jnp.int32(2**31 - 1), j)
        for m, j in zip(masks, tops)
    )
    return found, rest


def _for_rows(masks, fn, peel=0):
    def call(found):
        for valid, row in found:
            pl.when(valid)(functools.partial(fn, row))

    first = []
    for _ in range(peel):
        found, masks = _pop_rows(masks)
        first += found
    call(first)

    def step(ms):
        found, rest = _pop_rows(ms)
        call(found)
        return rest

    lax.while_loop(lambda ms: (ms[0] | ms[1]) != 0, step, tuple(masks))


def _moe(
    x_hbm, router_hbm, route_hbm, expert_hbm, shared_hbm,
    o_ref,
    x_v, router_v, route_v, expert_v, shared_v, send_buf, recv_buf,
    load_sems, send_sem, recv_sem,
):
    n_tok = x_v.shape[0]
    n_exp = router_v.shape[0]
    rows, half = recv_buf.shape
    part = rows // 2

    def load(i, src, dst):
        copy = pltpu.make_async_copy(src, dst, load_sems.at[i])
        copy.start()
        return copy

    head, tail = pl.ds(0, rows), pl.ds(rows, n_tok - rows)
    route_in = load(0, route_hbm, route_v)
    head_in = load(1, x_hbm.at[head], x_v.at[head])
    expert_in = [
        load(2 + e, expert_hbm.at[e], expert_v.at[e]) for e in range(N_LOCAL)
    ]
    rest_in = [
        load(2 + N_LOCAL, x_hbm.at[tail], x_v.at[tail]),
        load(3 + N_LOCAL, shared_hbm, shared_v),
        load(4 + N_LOCAL, router_hbm, router_v),
    ]

    me = lax.axis_index("i")
    barrier = pltpu.get_barrier_semaphore()
    for k in range(1, N_DEV):
        pl.semaphore_signal(
            barrier, inc=1,
            device_id=((me + k) & (N_DEV - 1),), device_id_type=MESH,
        )

    sub = lax.broadcasted_iota(jnp.int32, (8, 128), 0)
    lane = lax.broadcasted_iota(jnp.int32, (8, 128), 1)
    bit = (jnp.int32(1) << (15 - (lane & 15))).astype(jnp.float32)
    in_word = (lane >> 5) == (sub >> 1)
    bit_hi = jnp.where(in_word & ((lane & 16) == 0), bit, 0.0)
    bit_lo = jnp.where(in_word & ((lane & 16) != 0), bit, 0.0)
    wanted = me * N_LOCAL + (sub & 1)
    route_in.wait()
    masks = [[] for _ in range(N_LOCAL)]
    for h in range(n_tok // 128):
        route = route_v[:, pl.ds(128 * h, 128)] & (n_exp - 1)
        hit = jnp.broadcast_to(route, (8, 128)) == wanted
        hi, lo = (
            jnp.sum(jnp.where(hit, b, 0.0), axis=1, keepdims=True).astype(jnp.int32)
            for b in (bit_hi, bit_lo)
        )
        words = (hi << 16) | lo
        for s in range(8):
            masks[s & 1].append(words[s, 0])

    def remote_rows(chip, e, action, peel=0):
        def fn(t):
            action(pltpu.make_async_remote_copy(
                src_ref=send_buf.at[pl.ds(e * n_tok + chip * rows + t, 1)],
                dst_ref=recv_buf.at[pl.ds(t, 1)],
                send_sem=send_sem, recv_sem=recv_sem,
                device_id=(chip,), device_id_type=MESH,
            ))

        theirs = masks[e][2 * chip:2 * chip + 2]
        _for_rows([jnp.where(me == chip, 0, m) for m in theirs], fn, peel)

    def local_rows():
        def fn(e, t):
            pltpu.make_async_copy(
                send_buf.at[pl.ds(e * n_tok + me * rows + t, 1)],
                recv_buf.at[pl.ds(t, 1)],
                recv_sem,
            ).start()

        for e in range(N_LOCAL):
            own = masks[e][:2]
            for chip in range(1, N_DEV):
                own = [
                    jnp.where(me == chip, masks[e][2 * chip + w], own[w])
                    for w in range(2)
                ]
            _for_rows(own, functools.partial(fn, e))

    @pl.when(me != 0)
    def _():
        pl.semaphore_wait(barrier, N_DEV - 1)

    head_in.wait()
    x_head = [x_v[pl.ds(j * part, part), :].astype(jnp.bfloat16) for j in range(2)]
    for e in range(N_LOCAL):
        expert_in[e].wait()
        for j in range(2):
            send_buf[pl.ds(e * n_tok + j * part, part), :] = _pack(
                _mm(x_head[j], expert_v[e])
            )
        remote_rows(0, e, lambda copy: copy.start(), peel=6)

    for copy in rest_in:
        copy.wait()
    for e in range(N_LOCAL):
        send_buf[pl.ds(e * n_tok + rows, n_tok - rows), :] = _pack(
            _mm(x_v[tail, :], expert_v[e])
        )

    x_own = [
        x_v[pl.ds(pl.multiple_of(me * rows + j * part, part), part), :]
        for j in range(2)
    ]
    shared = jnp.concatenate([_mm(v, shared_v[...]) for v in x_own], axis=0)
    scores = jnp.concatenate(
        [
            lax.dot_general(
                v, router_v[...], (((1,), (1,)), ((), ())),
                precision=lax.Precision.HIGHEST,
                preferred_element_type=jnp.float32,
            )
            for v in x_own
        ],
        axis=0,
    )
    probs = jnp.exp(scores - jnp.max(scores, axis=-1, keepdims=True))
    route = (route_v[...] & (n_exp - 1)).astype(jnp.float32)
    row = lax.broadcasted_iota(jnp.int32, (rows, n_tok), 0)
    tok = lax.broadcasted_iota(jnp.int32, (rows, n_tok), 1)
    chosen = jnp.sum(
        jnp.where(tok == row + me * rows, route, 0.0), axis=-1, keepdims=True
    )
    expert = lax.broadcasted_iota(jnp.int32, scores.shape, 1).astype(jnp.float32)
    gate = jnp.sum(
        jnp.where(expert == chosen, probs, 0.0), axis=-1, keepdims=True
    ) / jnp.sum(probs, axis=-1, keepdims=True)
    gate = jnp.broadcast_to(gate, (rows, half))

    @pl.when(me == 0)
    def _():
        local_rows()
        pl.semaphore_wait(barrier, N_DEV - 1)

    for chip in (1, 3, 2):
        for e in range(N_LOCAL):
            remote_rows(chip, e, lambda copy: copy.start())
    pl.when(me != 0)(local_rows)
    for chip in range(N_DEV):
        for e in range(N_LOCAL):
            remote_rows(chip, e, lambda copy: copy.wait_send())

    pltpu.make_async_copy(recv_buf, recv_buf, recv_sem).wait()
    lo, hi = _unpack(recv_buf[...])
    o_ref[:, :half] = shared[:, :half] + gate * lo
    o_ref[:, half:] = shared[:, half:] + gate * hi


def _moe_body(*refs):
    pl.run_scoped(
        functools.partial(_moe, *refs),
        pltpu.SemaphoreType.DMA((5 + N_LOCAL,)),
        pltpu.SemaphoreType.DMA,
        pltpu.SemaphoreType.DMA,
    )


def pallas_dist_moe_shared_ep_outshard_n256_d128_e2_h256_kernel(
    x: jax.Array,
    router_W: jax.Array,
    route_idx: jax.Array,
    expert_W: jax.Array,
    shared_W: jax.Array,
):
    n_tok, d = x.shape
    n_exp = router_W.shape[1]
    n_local, _, h = expert_W.shape
    rows = n_tok // N_DEV
    assert (rows, n_local, n_exp, h) == (2 * WORD, N_LOCAL, N_LOCAL * N_DEV, 256)

    return pl.pallas_call(
        _moe_body,
        out_shape=jax.ShapeDtypeStruct((rows, h), jnp.float32),
        in_specs=[pl.BlockSpec(memory_space=pl.ANY)] * 5,
        out_specs=pl.BlockSpec(memory_space=pltpu.VMEM),
        scratch_shapes=[
            pltpu.VMEM((n_tok, d), jnp.float32),
            pltpu.VMEM((n_exp, d), jnp.float32),
            pltpu.VMEM((1, n_tok), jnp.int32),
            pltpu.VMEM((N_LOCAL, d, h), jnp.float32),
            pltpu.VMEM((d, h), jnp.float32),
            pltpu.VMEM((N_LOCAL * n_tok, h // 2), jnp.uint32),
            pltpu.VMEM((rows, h // 2), jnp.uint32),
        ],
        compiler_params=pltpu.CompilerParams(collective_id=0),
    )(x, router_W.T, route_idx.reshape(1, n_tok), expert_W, shared_W)
```
